```python
import numpy as np
kernel_name = 'dist_attn_self_mha_htp_b1_sq256_skv256_d1024_hq8_dh128'

def setup_inputs():
    x = np.random.randn(1, 256, 1024).astype(np.float32)
    Wq = np.random.randn(1024, 4096).astype(np.float32) * 0.02
    Wk = np.random.randn(1024, 4096).astype(np.float32) * 0.02
    Wv = np.random.randn(1024, 4096).astype(np.float32) * 0.02
    Wo = np.random.randn(4096, 1024).astype(np.float32) * 0.02
    return {'x': x, 'Wq': Wq, 'Wk': Wk, 'Wv': Wv, 'Wo': Wo}

def reference(x, Wq, Wk, Wv, Wo):
    B, Sq, Hq, Hkv, Dh = (1, 256, 32, 32, 128)
    Q = (x @ Wq).reshape(B, Sq, Hq, Dh)
    K = (x @ Wk).reshape(B, Sq, Hkv, Dh)
    V = (x @ Wv).reshape(B, Sq, Hkv, Dh)
    Skv = K.shape[1]
    out = np.zeros((B, Sq, Hq, Dh), dtype=np.float32)
    m = np.full((B, Hq, Sq, 1), -np.inf, dtype=np.float32)
    l = np.zeros((B, Hq, Sq, 1), dtype=np.float32)
    for j0 in range(0, Skv, 256):
        Kj = K[:, j0:j0 + 256].copy()
        Vj = V[:, j0:j0 + 256].copy()
        sj = np.einsum('bihd,bjhd->bhij', Q, Kj).astype(np.float32) * 0.08838834764831843
        mj = sj.max(axis=-1, keepdims=True)
        m_new = np.maximum(m, mj)
        alpha = np.exp(m - m_new)
        pj = np.exp(sj - m_new)
        l = l * alpha + pj.sum(axis=-1, keepdims=True)
        out = out * alpha.transpose(0, 2, 1, 3) + np.einsum('bhij,bjhd->bihd', pj, Vj)
        m = m_new
    out = (out / l.transpose(0, 2, 1, 3)).reshape(B, Sq, Hq * Dh)
    return out @ Wo
```

```python
import jax
import jax.numpy as jnp
from jax import lax
from jax.experimental import pallas as pl
from jax.experimental.pallas import tpu as pltpu

BF = jnp.bfloat16
F32 = jnp.float32
S = 256
D = 1024
H = 8
DH = 128
SCALE = 0.08838834764831843
NC = 8
CW = D // NC
RG = 64
OUT_DT = F32
SCOPES = False
LPRIO = 0
NOCHK = True

import contextlib
def scope(n):
    return jax.named_scope(n) if SCOPES else contextlib.nullcontext()


def pallas_dist_attn_self_mha_htp_b1_sq256_skv256_d1024_hq8_dh128_kernel(x, Wq, Wk, Wv, Wo):
    loads = [
        ("qa", 0, 0, 1024, 0, 512), ("ka", 1, 0, 1024, 0, 512),
        ("qb", 0, 0, 1024, 512, 512), ("kb", 1, 0, 1024, 512, 512),
        ("va1", 2, 0, 512, 0, 512), ("va2", 2, 512, 512, 0, 512),
        ("vb1", 2, 0, 512, 512, 384), ("vb2", 2, 512, 512, 512, 384),
        ("vc", 2, 0, 1024, 896, 128),
    ] + [("o%d" % c, 3, 0, 1024, c * CW, CW) for c in range(NC)]

    def body(x_hbm, wq_hbm, wk_hbm, wv_hbm, wo_hbm, out_ref,
             xf, w, xb, qb, kb, pb, vacc, vb, ob, part, sb1, rb1, sb2, rb2, sb3, rb3,
             lsem, ssem, rsem):
        me = lax.axis_index("i")
        hbm = (wq_hbm, wk_hbm, wv_hbm, wo_hbm)
        xcp = pltpu.make_async_copy(x_hbm.at[0], xf, lsem.at[len(loads)])
        xcp.start(priority=LPRIO)
        cps = {}
        for j, (nm, i, r0, nr, c0, nc) in enumerate(loads):
            cp = pltpu.make_async_copy(hbm[i].at[pl.ds(r0, nr), pl.ds(c0, nc)],
                                       w.at[i, pl.ds(r0, nr), pl.ds(c0, nc)], lsem.at[j])
            cp.start(priority=LPRIO)
            cps[nm] = cp
        left = (me + 3) % 4
        right = (me + 1) % 4
        bs = pltpu.get_barrier_semaphore()
        for nb in (left, right):
            pl.semaphore_signal(bs, inc=1, device_id=(nb,), device_id_type=pl.DeviceIdType.MESH)

        with scope("x"):
            xcp.wait()
            xb[...] = xf[...].astype(BF)

        def proj(i, r0, nr, c0, nc):
            return jnp.dot(xb[:, r0:r0 + nr], w[i, r0:r0 + nr, c0:c0 + nc].astype(BF),
                           preferred_element_type=F32)

        def scores(h):
            q = qb[:, h * DH:(h + 1) * DH]
            k = kb[:, h * DH:(h + 1) * DH]
            s = lax.dot_general(q, k, (((1,), (1,)), ((), ())), preferred_element_type=F32)
            m = jnp.max(s, axis=-1, keepdims=True)
            p = jnp.exp(s - m)
            l = jnp.sum(p, axis=-1, keepdims=True)
            pb[h] = (p * (1.0 / l)).astype(BF)

        def pv(h):
            ob[:, h * DH:(h + 1) * DH] = jnp.dot(
                pb[h], vb[:, h * DH:(h + 1) * DH], preferred_element_type=F32).astype(BF)

        for half, c0 in (("a", 0), ("b", 512)):
            with scope("q" + half):
                cps["q" + half].wait()
                qb[:, c0:c0 + 512] = (proj(0, 0, 1024, c0, 512) * SCALE).astype(BF)
            with scope("k" + half):
                cps["k" + half].wait()
                kb[:, c0:c0 + 512] = proj(1, 0, 1024, c0, 512).astype(BF)
            with scope("s" + half):
                for h in range(c0 // DH, c0 // DH + 4):
                    scores(h)
        with scope("va1"):
            cps["va1"].wait()
            vacc[:, 0:512] = proj(2, 0, 512, 0, 512)
        with scope("va2"):
            cps["va2"].wait()
            vb[:, 0:512] = (vacc[:, 0:512] + proj(2, 512, 512, 0, 512)).astype(BF)
            for h in range(4):
                pv(h)
        with scope("vb1"):
            cps["vb1"].wait()
            vacc[:, 512:896] = proj(2, 0, 512, 512, 384)
        with scope("vb2"):
            cps["vb2"].wait()
            vb[:, 512:896] = (vacc[:, 512:896] + proj(2, 512, 512, 512, 384)).astype(BF)
            for h in range(4, 7):
                pv(h)
        with scope("vc"):
            cps["vc"].wait()
            vb[:, 896:1024] = proj(2, 0, 1024, 896, 128).astype(BF)
            pv(7)
        pl.semaphore_wait(bs, 2)

        def rows(a):
            return pl.ds(pl.multiple_of((a % 4) * RG, RG), RG)

        def rdma(src, dst, step, c, d, tgt):
            return pltpu.make_async_remote_copy(
                src_ref=src, dst_ref=dst, send_sem=ssem.at[step, c, d], recv_sem=rsem.at[step, c, d],
                device_id=(tgt,), device_id_type=pl.DeviceIdType.MESH)

        def s1(c):
            return (rdma(sb1.at[c, 0], rb1.at[c, 0], 0, c, 0, right),
                    rdma(sb1.at[c, 1], rb1.at[c, 1], 0, c, 1, left))

        def s2(c):
            return (rdma(sb2.at[c, 0], rb2.at[c, 0], 1, c, 0, right),
                    rdma(sb2.at[c, 1], rb2.at[c, 1], 1, c, 1, left))

        def s3(c):
            return (rdma(sb3.at[c, 0], rb3.at[c, 0], 2, c, 0, right),
                    rdma(sb3.at[c, 1], rb3.at[c, 1], 2, c, 1, left))

        def act0(c):
            cps["o%d" % c].wait()
            part[c] = jnp.dot(ob[...], w[3, :, c * CW:(c + 1) * CW].astype(BF), preferred_element_type=F32)
            sb1[c, 0] = part[c, rows(me + 1), :].astype(BF)
            sb1[c, 1] = part[c, rows(me + 2), :].astype(BF)
            for cp in s1(c):
                cp.start()

        def act1(c):
            a, b = s1(c)
            n0, n1 = s2(c)
            a.wait_recv()
            t = part[c, rows(me), :] + rb1[c, 0].astype(F32)
            part[c, rows(me), :] = t
            sb2[c, 0] = t.astype(BF)
            n0.start()
            b.wait_recv()
            t = part[c, rows(me + 3), :] + rb1[c, 1].astype(F32)
            part[c, rows(me + 3), :] = t
            sb2[c, 1] = t.astype(BF)
            n1.start()

        def act2(c):
            a, b = s2(c)
            n0, n1 = s3(c)
            a.wait_recv()
            t = part[c, rows(me + 3), :] + rb2[c, 0].astype(F32)
            sb3[c, 0] = t.astype(BF)
            n0.start()
            out_ref[0, rows(me + 3), c * CW:(c + 1) * CW] = t.astype(OUT_DT)
            b.wait_recv()
            t = part[c, rows(me), :] + rb2[c, 1].astype(F32)
            sb3[c, 1] = t.astype(BF)
            n1.start()
            out_ref[0, rows(me), c * CW:(c + 1) * CW] = t.astype(OUT_DT)

        def act3(c):
            a, b = s3(c)
            a.wait_recv()
            out_ref[0, rows(me + 2), c * CW:(c + 1) * CW] = rb3[c, 0].astype(OUT_DT)
            b.wait_recv()
            out_ref[0, rows(me + 1), c * CW:(c + 1) * CW] = rb3[c, 1].astype(OUT_DT)

        LAG = 2
        for t in range(NC + 2 * LAG):
            if 0 <= t - 2 * LAG < NC:
                with scope("a2_%d" % (t - 2 * LAG)):
                    act2(t - 2 * LAG)
            if 0 <= t - LAG < NC:
                with scope("a1_%d" % (t - LAG)):
                    act1(t - LAG)
            if t < NC:
                with scope("a0_%d" % t):
                    act0(t)
        for c in range(NC):
            with scope("a3_%d" % c):
                act3(c)
        with scope("fin"):
            for c in range(NC):
                for st in (s1, s2, s3):
                    for cp in st(c):
                        cp.wait_send()

    cbuf = pltpu.VMEM((NC, 2, RG, CW), BF)
    return pl.pallas_call(
        body,
        out_shape=jax.ShapeDtypeStruct((1, S, D), OUT_DT),
        in_specs=[pl.BlockSpec(memory_space=pl.ANY)] * 5,
        out_specs=pl.BlockSpec(memory_space=pltpu.VMEM),
        scratch_shapes=[
            pltpu.VMEM((S, D), F32), pltpu.VMEM((4, D, D), F32),
            pltpu.VMEM((S, D), BF), pltpu.VMEM((S, D), BF), pltpu.VMEM((S, D), BF),
            pltpu.VMEM((H, S, S), BF), pltpu.VMEM((S, D), F32), pltpu.VMEM((S, D), BF),
            pltpu.VMEM((S, D), BF), pltpu.VMEM((NC, S, CW), F32),
            cbuf, cbuf, cbuf, cbuf, cbuf, cbuf,
            pltpu.SemaphoreType.DMA((len(loads) + 1,)),
            pltpu.SemaphoreType.DMA((3, NC, 2)), pltpu.SemaphoreType.DMA((3, NC, 2)),
        ],
        compiler_params=pltpu.CompilerParams(collective_id=0, vmem_limit_bytes=48 * 2**20,
            disable_semaphore_checks=NOCHK, disable_bounds_checks=NOCHK),
    )(x, Wq, Wk, Wv, Wo)
```

```python
import jax
import jax.numpy as jnp
from jax import lax
from jax.experimental import pallas as pl
from jax.experimental.pallas import tpu as pltpu

BF = jnp.bfloat16
F32 = jnp.float32
S = 256
D = 1024
H = 8
DH = 128
QSCALE = 0.08838834764831843 * 1.4426950408889634
NC = 8
CW = D // NC
PPC = 4
RG = S // PPC
G = 32
FULL = 15
ALL = slice(None)
BORD = (2, 1, 3, 0)

XSEND = ((1, 0), (3, 4), (1, 1), (3, 5), (1, 2), (3, 6), (1, 3), (3, 7), (1, 7), (3, 3), (1, 6), (3, 2))
XFWD = {1: {0: 2, 1: 2, 2: 2, 3: 2}, 2: {0: 3, 1: 3, 4: 1, 5: 1}, 3: {4: 2, 5: 2, 6: 2, 7: 2}}
KORD = ((0, 1, 2, 3, 4, 5, 6, 7), (0, 1, 2, 3, 4, 7, 5, 6),
        (0, 4, 1, 5, 2, 6, 3, 7), (4, 5, 6, 7, 0, 3, 1, 2))
SWEEP = ((0, 1), (2,), (3,), (4,), (5,))

PLAIN = ((ALL,) * 4,)
B3 = ((0, ALL, ALL, ALL), (1, ALL, ALL, ALL))
B01 = tuple((ALL, ALL, a, b) for a in range(2) for b in range(2))
BS = ((0,) + B3[0], (1,) + B3[0], B3[1])
VP = ((0, 4, 0, 2, B3), (0, 4, 2, 2, B3), (0, 4, 4, 2, B3), (0, 4, 6, 2, B3), (4, 4, 0, 2, B3),
      (4, 4, 2, 2, BS), (4, 4, 4, 1, PLAIN), (4, 4, 5, 1, PLAIN), (4, 2, 6, 2, B01), (6, 2, 6, 2, B01))
SIDE = (("q", 0, 48), ("q", 1, 48), ("v", 5, 1))
STEPS = ("Q0 Q1 q0 q1 Q2 s0 s1 q2 Q3 s2 s3 q3 B2 V0 s4 s5 v0 V1 s6 s7 v1 V2 v2 I2 I3 I4 I5 "
         "V3 v3 p0 p1 p2 p3 V4 v4 V5 v5 V6 v6 V7 v7 V8 v8 V9 v9 p4 p5 p6 p7")
OISS = {1: 6, 2: 7}

MODES = (1,3,3,3,3,3,2,2)
PIECES = ((0,0,0,32),(0,0,32,32),(0,1,0,64),(0,2,0,32),(0,2,32,32),(0,3,0,64),(1,0,0,32),(1,0,32,32),(1,1,0,64),(1,2,0,64),(1,3,0,32),(1,3,32,32),(2,0,0,64),(2,1,0,32),(2,1,32,32),(2,2,0,64),(2,3,0,64),(3,0,0,32),(3,0,32,32),(3,1,0,64),(3,2,0,64),(3,3,0,64),(4,0,0,32),(4,0,32,32),(4,1,0,32),(4,1,32,32),(4,2,0,32),(4,2,32,32),(4,3,0,32),(4,3,32,32),(5,0,0,64),(5,1,0,64),(5,2,0,32),(5,2,32,32),(5,3,0,32),(5,3,32,32),(6,0,0,64),(6,1,0,64),(6,2,0,32),(6,2,32,32),(6,3,0,64),(7,0,0,64),(7,1,0,64),(7,2,0,64),(7,3,0,32),(7,3,32,32))
ORD = ((7,0,4,3,6,2,1,5),(1,7,5,6,3,4,2,0),(5,1,3,7,2,6,0,4),(3,2,5,0,1,7,4,6))
PLANS = (((0,1,1,(-1,)),(3,2,8,(-1,)),(2,1,12,(-1,1)),(1,2,15,(-1,0,2)),(1,0,14,(-1,2)),(2,3,15,(3,))),((0,3,1,(-1,)),(3,2,9,(-1,0)),(2,1,13,(-1,1)),(1,2,15,(-1,2)),(1,0,15,(-1,2)),(0,3,15,(4,))),((0,1,1,(-1,)),(1,2,3,(-1,0)),(2,3,7,(-1,1)),(3,2,8,(-1,)),(2,1,12,(-1,3)),(1,0,14,(-1,4))),((0,3,1,(-1,)),(1,2,2,(-1,)),(3,2,9,(-1,0)),(2,1,13,(-1,2)),(1,0,15,(-1,3)),(0,3,15,(4,))),((0,1,1,(-1,)),(1,2,3,(-1,0)),(2,3,7,(-1,1)),(3,2,8,(-1,)),(2,1,12,(-1,3)),(1,0,15,(-1,0,4))),((0,3,1,(-1,)),(1,2,2,(-1,)),(2,3,6,(-1,1)),(3,2,9,(-1,0)),(2,1,13,(-1,3)),(1,0,15,(-1,4))),((2,1,4,(-1,)),(1,0,6,(-1,0)),(0,3,7,(-1,1)),(3,0,8,(-1,)),(0,1,9,(-1,3)),(1,2,11,(-1,4))),((1,0,2,(-1,)),(0,3,3,(-1,0)),(2,3,4,(-1,)),(3,0,12,(-1,2)),(0,1,13,(-1,3)),(3,2,11,(-1,1))),((1,0,2,(-1,)),(0,3,3,(-1,0)),(2,3,4,(-1,)),(3,0,12,(-1,2)),(3,2,11,(-1,1)),(2,1,15,(-1,4))),((1,0,2,(-1,)),(0,3,3,(-1,0)),(2,3,4,(-1,)),(3,0,12,(-1,2)),(0,1,13,(-1,3)),(3,2,15,(-1,1,2))),((1,0,2,(-1,)),(0,3,3,(-1,0)),(2,3,4,(-1,)),(3,0,12,(-1,2)),(0,1,13,(-1,3)),(3,2,11,(-1,1))),((1,0,2,(-1,)),(0,3,3,(-1,0)),(2,3,4,(-1,)),(3,0,12,(-1,2)),(3,2,15,(-1,1,2)),(2,1,15,(4,))),((0,1,1,(-1,)),(1,2,3,(-1,0)),(2,3,7,(-1,1)),(3,2,8,(-1,)),(2,1,12,(-1,3)),(1,0,15,(-1,0,4))),((2,1,4,(-1,)),(1,0,6,(-1,0)),(0,3,7,(-1,1)),(3,0,8,(-1,)),(0,1,15,(-1,1,3)),(3,2,15,(-1,2))),((0,1,1,(-1,)),(3,2,8,(-1,)),(2,1,12,(-1,1)),(1,0,14,(-1,2)),(0,3,15,(-1,3)),(3,2,15,(4,))),((0,1,1,(-1,)),(3,2,8,(-1,)),(2,1,12,(-1,1)),(1,0,14,(-1,2)),(0,3,15,(-1,3)),(3,2,15,(4,))),((0,1,1,(-1,)),(3,2,8,(-1,)),(2,1,12,(-1,1)),(1,2,15,(-1,0,2)),(1,0,15,(-1,0,2)),(0,3,15,(4,))),((0,1,1,(-1,)),(1,2,3,(-1,0)),(2,3,7,(-1,1)),(3,2,8,(-1,)),(2,1,12,(-1,3)),(1,0,15,(-1,0,4))),((2,1,4,(-1,)),(1,0,6,(-1,0)),(0,3,7,(-1,1)),(3,0,8,(-1,)),(0,1,9,(-1,3)),(1,2,15,(-1,0,4))),((2,1,4,(-1,)),(1,0,6,(-1,0)),(0,3,7,(-1,1)),(3,0,8,(-1,)),(0,1,9,(-1,3)),(1,2,11,(-1,4))),((0,1,1,(-1,)),(1,2,3,(-1,0)),(3,2,8,(-1,)),(2,3,15,(-1,1,2)),(2,1,12,(-1,2)),(1,0,15,(-1,0,4))),((2,1,4,(-1,)),(1,0,6,(-1,0)),(3,0,8,(-1,)),(0,1,9,(-1,2)),(0,3,15,(-1,1,2)),(1,2,15,(-1,0,3))),((0,1,1,(-1,)),(1,2,3,(-1,0)),(3,2,8,(-1,)),(2,3,15,(-1,1,2)),(2,1,15,(-1,1,2)),(3,0,15,(3,))),((0,1,1,(-1,)),(1,2,3,(-1,0)),(2,3,7,(-1,1)),(3,0,15,(-1,2)),(3,2,8,(-1,)),(2,1,15,(-1,1,4))),((0,3,1,(-1,)),(1,2,2,(-1,)),(2,3,6,(-1,1)),(3,0,15,(-1,0,2)),(3,2,9,(-1,0)),(2,1,13,(-1,4))),((0,3,1,(-1,)),(1,2,2,(-1,)),(2,3,6,(-1,1)),(3,0,15,(-1,0,2)),(0,1,15,(3,)),(3,2,9,(-1,0))),((0,3,1,(-1,)),(1,2,2,(-1,)),(2,3,6,(-1,1)),(3,2,9,(-1,0)),(2,1,13,(-1,3)),(1,0,15,(-1,4))),((0,1,1,(-1,)),(1,2,3,(-1,0)),(2,3,7,(-1,1)),(3,0,15,(-1,2)),(3,2,8,(-1,)),(2,1,15,(-1,1,4))),((0,3,1,(-1,)),(1,2,2,(-1,)),(2,3,6,(-1,1)),(3,0,14,(-1,2)),(3,2,9,(-1,0)),(2,1,15,(-1,1,4))),((0,3,1,(-1,)),(1,2,2,(-1,)),(3,2,9,(-1,0)),(2,3,15,(-1,1,2)),(2,1,13,(-1,2)),(1,0,15,(-1,4))),((1,0,2,(-1,)),(2,3,4,(-1,)),(3,0,12,(-1,1)),(0,3,15,(-1,0,2)),(3,2,15,(3,)),(2,1,15,(4,))),((2,1,4,(-1,)),(1,0,6,(-1,0)),(3,0,8,(-1,)),(0,1,9,(-1,2)),(1,2,11,(-1,3)),(2,3,15,(-1,4))),((1,0,2,(-1,)),(2,3,4,(-1,)),(3,0,12,(-1,1)),(0,3,15,(-1,0,2)),(3,2,15,(3,)),(2,1,15,(4,))),((2,1,4,(-1,)),(1,0,6,(-1,0)),(3,0,8,(-1,)),(0,1,15,(-1,1,2)),(0,3,15,(-1,1,2)),(1,2,15,(3,))),((2,1,4,(-1,)),(1,0,6,(-1,0)),(3,0,8,(-1,)),(0,1,9,(-1,2)),(0,3,15,(-1,1,2)),(3,2,15,(4,))),((2,1,4,(-1,)),(1,0,6,(-1,0)),(3,0,8,(-1,)),(0,1,9,(-1,2)),(1,2,11,(-1,3)),(2,3,15,(-1,4))),((0,3,1,(-1,)),(1,2,2,(-1,)),(2,3,6,(-1,1)),(3,0,15,(-1,0,2)),(0,1,15,(3,)),(3,2,15,(-1,0,2))),((0,3,1,(-1,)),(1,2,2,(-1,)),(2,3,6,(-1,1)),(3,0,14,(-1,2)),(3,2,9,(-1,0)),(2,1,13,(-1,4))),((1,0,2,(-1,)),(0,3,3,(-1,0)),(2,3,4,(-1,)),(3,0,12,(-1,2)),(3,2,15,(-1,1,2)),(2,1,15,(4,))),((0,3,1,(-1,)),(1,2,2,(-1,)),(2,3,6,(-1,1)),(3,0,14,(-1,2)),(3,2,15,(-1,0,2)),(2,1,15,(4,))),((0,3,1,(-1,)),(1,2,2,(-1,)),(2,3,6,(-1,1)),(3,0,15,(-1,0,2)),(0,1,15,(3,)),(1,2,15,(4,))),((0,3,1,(-1,)),(1,2,2,(-1,)),(2,3,6,(-1,1)),(3,0,15,(-1,0,2)),(0,1,15,(3,)),(3,2,15,(-1,0,2))),((0,3,1,(-1,)),(1,2,2,(-1,)),(2,3,6,(-1,1)),(3,0,15,(-1,0,2)),(0,1,15,(3,)),(3,2,9,(-1,0))),((0,1,1,(-1,)),(1,2,3,(-1,0)),(2,3,7,(-1,1)),(3,0,15,(-1,2)),(0,1,15,(3,)),(3,2,8,(-1,))),((0,1,1,(-1,)),(1,2,3,(-1,0)),(2,3,7,(-1,1)),(3,0,15,(-1,2)),(3,2,8,(-1,)),(2,1,15,(-1,1,4))),((1,0,2,(-1,)),(0,3,3,(-1,0)),(2,3,4,(-1,)),(3,0,12,(-1,2)),(0,1,15,(-1,0,3)),(1,2,15,(4,))))
FINS = (((-1,4),(-1,0,2),(3,),(5,)),((4,),(-1,2),(3,),(5,)),((-1,5),(-1,0,4),(-1,1,3),(-1,2)),((4,),(-1,3),(-1,1,2),(5,)),((5,),(-1,0,4),(-1,1,3),(-1,2)),((5,),(-1,4),(-1,1,3),(-1,0,2)),((-1,1,3),(-1,0,4),(-1,5),(-1,2)),((-1,0,3),(-1,4),(-1,5),(-1,1,2)),((-1,0,3),(5,),(-1,4),(-1,1,2)),((-1,0,3),(-1,4),(5,),(-1,1,2)),((-1,0,3),(-1,4),(-1,5),(-1,1,2)),((-1,0,3),(5,),(4,),(-1,1,2)),((5,),(-1,0,4),(-1,1,3),(-1,2)),((-1,1,3),(4,),(5,),(-1,2)),((-1,3),(-1,0,2),(5,),(4,)),((-1,3),(-1,0,2),(5,),(4,)),((4,),(-1,0,2),(3,),(5,)),((5,),(-1,0,4),(-1,1,3),(-1,2)),((-1,1,3),(-1,0,4),(5,),(-1,2)),((-1,1,3),(-1,0,4),(-1,5),(-1,2)),((5,),(-1,0,4),(-1,1,2),(3,)),((-1,1,2),(-1,0,3),(5,),(4,)),((5,),(4,),(-1,1,2),(3,)),((3,),(5,),(-1,1,4),(-1,2)),((3,),(-1,5),(-1,1,4),(-1,0,2)),((3,),(4,),(-1,1,5),(-1,0,2)),((5,),(-1,4),(-1,1,3),(-1,0,2)),((3,),(5,),(-1,1,4),(-1,2)),((-1,3),(5,),(-1,1,4),(-1,0,2)),((5,),(-1,4),(-1,1,2),(3,)),((-1,0,2),(5,),(4,),(3,)),((-1,1,2),(-1,0,3),(-1,4),(5,)),((-1,0,2),(5,),(4,),(3,)),((-1,1,2),(3,),(5,),(4,)),((-1,1,2),(-1,0,3),(5,),(4,)),((-1,1,2),(-1,0,3),(-1,4),(5,)),((3,),(4,),(5,),(-1,0,2)),((-1,3),(-1,5),(-1,1,4),(-1,0,2)),((-1,0,3),(5,),(4,),(-1,1,2)),((-1,3),(5,),(4,),(-1,0,2)),((3,),(4,),(5,),(-1,0,2)),((3,),(4,),(5,),(-1,0,2)),((3,),(4,),(-1,1,5),(-1,0,2)),((3,),(4,),(-1,1,5),(-1,2)),((3,),(5,),(-1,1,4),(-1,2)),((-1,0,3),(4,),(5,),(-1,1,2)))
SEQ = (((0,7,0),(3,43,0),(3,41,0),(1,44,0),(1,42,0),(4,0,0),(0,0,0),(3,2,0),(3,5,0),(1,4,0),(4,4,0),(1,1,0),(1,0,0),(1,3,0),(0,4,0),(3,23,0),(1,24,0),(1,27,0),(1,28,0),(4,3,0),(1,22,0),(1,25,0),(0,3,0),(3,17,0),(1,29,0),(1,20,0),(1,26,0),(4,6,0),(1,45,1),(1,19,4),(0,6,0),(3,39,0),(1,40,0),(1,18,4),(1,21,3),(4,2,0),(1,37,0),(0,2,0),(3,12,0),(1,16,0),(1,36,0),(4,1,0),(1,38,1),(1,14,0),(0,1,0),(1,7,1),(1,8,1),(1,6,4),(1,15,0),(4,5,0),(2,6,0),(2,8,0),(1,10,1),(1,9,1),(1,11,1),(1,9,4),(0,5,0),(2,9,0),(2,19,0),(2,10,0),(1,35,3),(2,11,0),(2,30,0),(2,31,0),(2,32,0),(2,33,0),(2,34,0),(2,35,0),(1,31,3),(2,21,0),(2,7,0),(1,30,3),(2,45,0),(1,34,3),(2,20,0),(1,32,3),(1,7,4),(2,17,0),(2,41,0),(1,34,4),(1,10,4),(2,18,0),(1,13,2),(1,13,4),(2,13,0),(1,33,4),(2,42,0),(1,45,4),(1,15,4),(2,44,0),(1,33,3),(2,15,0),(1,43,4),(1,16,5),(2,43,0),(2,16,0),(2,39,0),(1,42,4),(2,14,0),(1,14,4),(2,38,0),(1,18,2),(1,40,4),(2,12,0),(1,3,5),(2,40,0),(2,3,0),(1,19,2),(1,41,4),(2,4,0),(2,37,0),(2,1,0),(1,6,2),(1,36,4),(2,0,0),(1,1,5),(2,36,0),(1,21,4),(2,23,0),(2,2,0),(1,25,4),(5,43,0),(5,41,0),(5,44,0),(5,42,0),(5,2,0),(5,5,0),(5,4,0),(5,1,0),(5,0,0),(5,3,0),(5,23,0),(5,24,0),(5,27,0),(5,28,0),(5,22,0),(5,25,0),(5,17,0),(5,29,0),(5,26,0),(5,20,0),(5,45,1),(5,39,0),(5,19,4),(5,18,4),(5,40,0),(5,21,3),(5,37,0),(5,12,0),(5,36,0),(5,38,1),(5,16,0),(5,14,0),(5,7,1),(5,6,4),(5,8,1),(5,15,0),(5,10,1),(5,9,4),(5,9,1),(5,35,3),(5,11,1),(5,31,3),(5,30,3),(5,34,3),(5,32,3),(5,7,4),(5,34,4),(5,10,4),(5,13,2),(5,13,4),(5,33,4),(5,45,4),(5,33,3),(5,15,4),(5,43,4),(5,16,5),(5,14,4),(5,42,4),(5,18,2),(5,3,5),(5,40,4),(5,19,2),(2,28,0),(5,41,4),(5,6,2),(2,25,0),(2,5,0),(5,1,5),(2,22,0),(5,36,4),(2,26,0),(2,24,0),(5,25,4),(2,29,0),(5,21,4),(2,27,0)),((0,1,0),(3,8,0),(1,9,0),(1,7,0),(4,7,0),(0,7,0),(3,41,1),(1,11,0),(4,5,0),(1,42,1),(1,45,0),(1,10,0),(0,5,0),(3,32,0),(1,43,1),(1,30,0),(4,6,0),(1,34,1),(1,44,1),(0,6,0),(3,40,1),(3,38,0),(1,39,1),(1,35,1),(4,3,0),(1,31,1),(1,37,1),(1,6,1),(1,36,1),(0,3,0),(1,33,1),(4,4,0),(1,19,1),(1,17,1),(0,4,0),(3,28,1),(1,21,1),(1,23,1),(4,2,0),(1,22,1),(1,20,1),(1,20,5),(0,2,0),(2,20,0),(2,19,0),(2,18,0),(1,17,5),(1,25,1),(2,17,0),(1,18,1),(1,29,1),(1,13,1),(1,24,1),(4,0,0),(2,21,0),(1,15,3),(1,27,1),(1,12,1),(0,0,0),(1,16,4),(2,16,0),(1,2,1),(1,14,3),(2,14,0),(2,6,0),(1,12,5),(1,4,1),(2,12,0),(1,5,1),(2,15,0),(1,3,4),(2,3,0),(1,4,5),(2,1,0),(1,26,1),(2,9,0),(1,1,4),(2,4,0),(1,0,3),(2,35,0),(1,0,4),(2,0,0),(1,35,4),(1,2,5),(1,1,3),(2,31,0),(2,2,0),(1,31,4),(2,34,0),(1,5,5),(2,7,0),(2,5,0),(1,16,3),(2,10,0),(1,26,5),(2,22,0),(2,13,0),(1,29,5),(2,26,0),(1,45,5),(2,45,0),(2,29,0),(1,33,5),(2,33,0),(2,28,0),(1,19,5),(2,23,0),(2,43,0),(2,27,0),(1,18,5),(2,44,0),(1,3,1),(2,42,0),(1,6,5),(2,37,0),(1,40,5),(2,40,0),(2,8,0),(1,21,5),(5,8,0),(5,9,0),(5,7,0),(5,41,1),(5,11,0),(5,45,0),(5,42,1),(5,10,0),(5,32,0),(5,43,1),(5,30,0),(5,44,1),(5,34,1),(5,38,0),(5,40,1),(5,35,1),(5,39,1),(5,31,1),(5,37,1),(5,6,1),(5,33,1),(5,36,1),(5,17,1),(5,19,1),(5,28,1),(5,23,1),(5,21,1),(5,22,1),(5,20,5),(5,20,1),(5,17,5),(5,25,1),(5,18,1),(5,29,1),(5,13,1),(5,24,1),(5,27,1),(5,15,3),(5,12,1),(5,16,4),(5,14,3),(5,2,1),(5,4,1),(5,12,5),(5,3,4),(5,5,1),(5,4,5),(5,26,1),(5,1,4),(5,0,3),(5,0,4),(5,35,4),(5,1,3),(5,2,5),(5,31,4),(5,5,5),(5,26,5),(5,16,3),(5,29,5),(5,45,5),(5,33,5),(5,19,5),(5,18,5),(5,3,1),(2,41,0),(5,6,5),(2,38,0),(2,11,0),(2,36,0),(5,40,5),(2,39,0),(2,25,0),(5,21,5),(2,30,0),(2,24,0),(2,32,0)),((0,5,0),(3,30,1),(3,34,0),(3,35,0),(4,1,0),(1,31,0),(1,32,1),(0,1,0),(3,8,2),(1,6,0),(4,3,0),(1,9,2),(1,33,0),(0,3,0),(3,19,0),(1,10,2),(1,21,0),(1,20,4),(1,11,2),(1,7,2),(4,7,0),(0,7,0),(3,45,2),(1,41,2),(1,18,0),(1,42,2),(1,17,4),(4,2,0),(0,2,0),(3,13,0),(1,44,2),(1,15,2),(1,43,2),(4,6,0),(1,16,2),(1,14,2),(0,6,0),(3,38,2),(1,39,2),(1,40,2),(1,12,4),(4,0,0),(1,37,2),(0,0,0),(1,3,3),(1,36,2),(1,1,2),(1,4,4),(4,4,0),(2,44,0),(2,17,0),(1,0,2),(1,17,2),(1,2,4),(0,4,0),(2,43,0),(1,23,2),(2,42,0),(1,28,2),(1,5,4),(2,20,0),(1,25,2),(1,22,3),(1,22,4),(2,22,0),(1,24,2),(1,26,4),(2,23,0),(1,27,2),(1,29,4),(2,29,0),(2,27,0),(1,20,3),(1,28,5),(2,28,0),(1,23,5),(2,38,0),(2,12,0),(1,29,3),(1,27,5),(2,39,0),(1,2,2),(1,44,5),(2,2,0),(1,37,5),(2,37,0),(2,4,0),(1,4,2),(1,5,2),(1,8,5),(2,8,0),(2,5,0),(2,26,0),(1,12,2),(1,38,5),(2,41,0),(2,0,0),(1,11,5),(2,11,0),(2,35,0),(1,35,5),(1,39,5),(2,1,0),(1,0,5),(1,30,5),(2,30,0),(1,26,2),(2,34,0),(2,31,0),(1,31,5),(1,24,5),(2,24,0),(1,32,5),(5,34,0),(5,30,1),(5,35,0),(5,32,1),(5,31,0),(5,6,0),(5,8,2),(5,33,0),(5,9,2),(5,10,2),(5,19,0),(5,11,2),(5,7,2),(5,21,0),(5,45,2),(5,20,4),(5,41,2),(5,18,0),(5,17,4),(5,42,2),(5,13,0),(5,44,2),(5,15,2),(5,43,2),(5,38,2),(5,16,2),(5,39,2),(5,14,2),(5,40,2),(5,12,4),(5,3,3),(5,37,2),(5,1,2),(5,4,4),(5,36,2),(5,0,2),(5,17,2),(5,23,2),(5,2,4),(5,28,2),(5,25,2),(5,5,4),(5,22,3),(5,22,4),(5,24,2),(5,26,4),(5,27,2),(5,29,4),(5,28,5),(5,20,3),(5,23,5),(5,29,3),(5,27,5),(5,44,5),(5,2,2),(5,4,2),(5,37,5),(5,5,2),(5,8,5),(5,38,5),(5,12,2),(5,11,5),(5,35,5),(5,39,5),(5,0,5),(2,32,0),(2,16,0),(5,26,2),(2,7,0),(5,30,5),(2,45,0),(5,24,5),(2,33,0),(5,31,5),(2,15,0),(5,32,5),(2,25,0),(2,19,0),(2,10,0),(2,18,0),(2,3,0),(2,36,0),(2,6,0),(2,13,0),(2,40,0),(2,9,0),(2,14,0),(2,21,0)),((0,3,0),(3,17,3),(3,20,2),(3,18,3),(1,21,2),(4,2,0),(0,2,0),(3,13,3),(3,16,1),(1,15,1),(1,19,3),(4,5,0),(0,5,0),(3,31,2),(1,12,3),(1,33,2),(4,0,0),(1,14,1),(1,35,2),(1,34,2),(0,0,0),(3,2,3),(1,30,2),(1,0,1),(4,1,0),(1,32,2),(1,5,3),(0,1,0),(3,6,3),(1,8,3),(1,3,2),(1,1,1),(1,4,3),(4,7,0),(1,9,3),(0,7,0),(3,44,4),(1,10,3),(1,11,3),(1,43,5),(4,4,0),(1,7,3),(1,45,3),(1,42,5),(0,4,0),(2,45,0),(1,41,3),(2,41,0),(1,27,4),(1,26,3),(4,6,0),(2,42,0),(1,22,2),(1,42,3),(1,23,4),(1,44,3),(1,29,2),(1,28,4),(0,6,0),(2,44,0),(1,43,3),(2,43,0),(1,38,4),(2,38,0),(1,39,3),(1,39,4),(2,39,0),(2,7,0),(1,38,3),(1,37,4),(1,40,3),(2,40,0),(2,8,0),(1,8,4),(2,10,0),(1,37,3),(2,37,0),(1,41,5),(2,9,0),(1,36,3),(2,36,0),(2,11,0),(1,11,4),(2,17,0),(1,23,3),(1,30,4),(2,23,0),(2,30,0),(1,28,3),(2,28,0),(2,32,0),(1,25,3),(1,34,5),(2,25,0),(2,34,0),(1,22,5),(1,24,4),(2,22,0),(2,13,0),(1,24,3),(1,32,4),(2,24,0),(2,33,0),(1,27,3),(1,7,5),(2,27,0),(1,15,5),(2,15,0),(2,20,0),(1,25,5),(2,29,0),(2,16,0),(1,10,5),(2,14,0),(1,36,5),(2,2,0),(2,18,0),(2,4,0),(2,3,0),(1,13,5),(1,9,5),(2,5,0),(2,19,0),(2,6,0),(1,14,5),(5,17,3),(5,18,3),(5,20,2),(5,21,2),(5,13,3),(5,16,1),(5,19,3),(5,15,1),(5,31,2),(5,12,3),(5,33,2),(5,14,1),(5,35,2),(5,34,2),(5,2,3),(5,0,1),(5,30,2),(5,32,2),(5,5,3),(5,6,3),(5,3,2),(5,1,1),(5,8,3),(5,4,3),(5,44,4),(5,9,3),(5,10,3),(5,43,5),(5,11,3),(5,7,3),(5,42,5),(5,45,3),(5,27,4),(5,26,3),(5,41,3),(5,22,2),(5,23,4),(5,42,3),(5,29,2),(5,44,3),(5,28,4),(5,38,4),(5,43,3),(5,39,4),(5,39,3),(5,38,3),(5,37,4),(5,40,3),(5,8,4),(5,37,3),(5,41,5),(5,11,4),(5,36,3),(5,23,3),(5,30,4),(5,28,3),(5,34,5),(5,25,3),(5,24,4),(5,22,5),(5,32,4),(5,24,3),(5,7,5),(5,27,3),(5,15,5),(5,25,5),(5,10,5),(5,36,5),(5,13,5),(2,12,0),(2,1,0),(2,35,0),(5,9,5),(2,0,0),(2,21,0),(5,14,5),(2,26,0),(2,31,0)))


def pallas_dist_attn_self_mha_htp_b1_sq256_skv256_d1024_hq8_dh128_kernel(x, Wq, Wk, Wv, Wo):
    rslot, sslot, nr, ns = {}, {}, [0] * 4, [0] * 4
    for p, msgs in enumerate(PLANS):
        for m, (src, dst, _, _) in enumerate(msgs):
            rslot[p, m], sslot[p, m] = nr[dst], ns[src]
            nr[dst] += 1
            ns[src] += 1
    side = {(kind, i): rows for kind, i, rows in SIDE}
    L_X, L_QK = 0, 1
    L_H = L_QK + len(SWEEP)
    L_V = L_H + 4
    L_O = L_V + len(VP)
    L_S = L_O + 2 * NC

    blocks = [(k, i) for k in range(NC) for i in ((0, 1) if MODES[k] >= 2 else (1,))]
    bpos = [[i for i, t in enumerate(SEQ[d]) if t[0] in (0, 4)] + [len(SEQ[d])] for d in range(4)]
    pos, early = {}, {}
    for d in range(4):
        for b, (k, last) in enumerate(blocks):
            first, early[d, b] = [], 0
            for t in SEQ[d][bpos[d][b] + 1:]:
                if t[0] != 3:
                    break
                if PIECES[t[1]][1] not in first:
                    first.append(PIECES[t[1]][1])
                early[d, b] += 1
            assert len(first) <= PPC // 2
            if last:
                for j, g in enumerate(first + [g for g in range(PPC) if g not in first]):
                    pos[d, ORD[d][k], g] = j

    xsends = [[(e, tgt) for tgt, e in XSEND]] + [sorted(XFWD[d].items()) for d in (1, 2, 3)]
    waits, sums, arrived, finished = {}, {}, set(), set()
    for d in range(4):
        for i, (kind, p, m) in enumerate(SEQ[d]):
            if kind in (1, 2, 3):
                deps = FINS[p][d] if kind == 2 else PLANS[p][m][3]
                total = kind == 2 or PLANS[p][m][2] == FULL
                waits[d, i] = [j for j in deps if j >= 0 and (p, j) not in arrived]
                arrived.update((p, j) for j in waits[d, i])
                sums[d, i] = deps if len(deps) > 1 and not (total and (d, p) in finished) else ()
                if total:
                    finished.add((d, p))
    assert len(arrived) == len(rslot) and len(finished) == 4 * len(PIECES)
    xdone = [[t[0] for t in SEQ[d]].index(5) for d in range(4)]

    def body(x_hbm, wq_hbm, wk_hbm, wv_hbm, wo_hbm, out_ref,
             xf, w, wv, wo, xb, acc, qb, kb, pb, vacc, vb, ob, pacc, part, partb, rbuf, sbuf,
             lsem, xssem, xrsem, ssem, rsem, *sms):
        me = lax.axis_index("i")

        def branches(fn, devs):
            for d in devs:
                pl.when(me == d)(lambda d=d: fn(d))

        def pick(vals):
            return jnp.where(me < 2, jnp.where(me == 0, vals[0], vals[1]),
                             jnp.where(me == 2, vals[2], vals[3]))

        def wait_all(ref, sem):
            pltpu.make_async_copy(ref, ref, sem).wait()

        def issue_qk(d, js, lo=0, hi=None):
            def slabs(sl):
                es = [KORD[d][t] for t in sl]
                if len(es) == 2 and es[1] == es[0] + 1:
                    return [(es[0] * 128, sl[0] * 128, 256)]
                return [(e * 128, t * 128, 128) for e, t in zip(es, sl)]

            todo = [None] if d == 0 and 0 in js else []
            todo += [(j, i) + sl for j in js for i in range(2) for sl in slabs(SWEEP[j])]
            for t in todo[lo:hi]:
                if t is None:
                    pltpu.make_async_copy(x_hbm.at[0], xf, lsem.at[L_X]).start()
                else:
                    j, i, r0, o, n = t
                    pltpu.make_async_copy((wq_hbm, wk_hbm)[i].at[pl.ds(r0, n), :],
                                          w.at[i, pl.ds(o, n), :], lsem.at[L_QK + j]).start()

        def issue_qk_last(d):
            for hf in range(2):
                for i in range(2):
                    for u in range(2):
                        for t in (6, 7):
                            cut = side["q", hf] if (i, u, t) == (0, 0, 6) else 0
                            pltpu.make_async_copy(
                                (wq_hbm, wk_hbm)[i].at[pl.ds(KORD[d][t] * 128 + u * 64 + cut, 64 - cut),
                                                       pl.ds(hf * 512, 512)],
                                w.at[hf, pl.ds(t * 128 + u * 64 + cut, 64 - cut), pl.ds(i * 512, 512)],
                                lsem.at[L_H + 2 * hf + i]).start()

        def vbox(n, sub=(ALL,) * 4):
            h0, nh, e0, ne, _ = VP[n]
            if len(sub) == 5:
                e0, ne, sub = e0 + sub[0], 1, sub[1:]
            return (pl.ds(e0, ne),) + sub + (ALL, pl.ds(h0 * DH, nh * DH))

        def issue_v():
            for n in range(len(VP)):
                for sub in VP[n][4][side.get(("v", n), 0):]:
                    pltpu.make_async_copy(wv_hbm.at[vbox(n, sub)], wv.at[vbox(n, sub)],
                                          lsem.at[L_V + n]).start()

        def issue_o(k):
            c0 = pl.multiple_of(pick([ORD[d][k] * CW for d in range(4)]), CW)
            for i in range(2):
                for a in range(2):
                    pltpu.make_async_copy(
                        wo_hbm.at[pl.ds(i * G // 2, G // 2), a, :, :, pl.ds(c0, CW)],
                        wo.at[k, pl.ds(i * G // 2, G // 2), a], lsem.at[L_O + 2 * k + i]).start()

        def side_refs(n):
            kind, i, rows = SIDE[n]
            if kind == "q":
                r0 = pl.multiple_of(pick([KORD[d][6] * 128 for d in range(4)]), 128)
                return (wq_hbm.at[pl.ds(r0, rows), pl.ds(i * 512, 512)],
                        w.at[i, pl.ds(768, rows), pl.ds(0, 512)], lsem.at[L_H + 2 * i])
            box = vbox(i, VP[i][4][0])
            return wv_hbm.at[box], wv.at[box], lsem.at[L_V + i]

        def side_in(n):
            return pltpu.make_async_copy(side_refs(n)[0], sms[n], lsem.at[L_S + n])

        def side_out(*ns):
            for n in ns:
                side_in(n).wait()
            for n in ns:
                pltpu.make_async_copy(sms[n], *side_refs(n)[1:]).start()

        branches(lambda d: issue_qk(d, range(4), 0, 1), BORD)
        barrier = pltpu.get_barrier_semaphore()
        for nb in ((me + 3) % 4, (me + 1) % 4):
            pl.semaphore_signal(barrier, inc=1, device_id=(nb,), device_id_type=pl.DeviceIdType.MESH)
        side_in(0).start()
        side_in(1).start()
        branches(lambda d: issue_qk(d, range(4), 1), range(4))

        def xcopy(e, tgt, slot):
            return pltpu.make_async_remote_copy(
                src_ref=xb.at[e], dst_ref=xb.at[e], send_sem=xssem.at[slot], recv_sem=xrsem.at[e],
                device_id=(tgt,), device_id_type=pl.DeviceIdType.MESH)

        def xsend(d, e, tgt):
            xcopy(e, tgt, xsends[d].index((e, tgt))).start()

        def xget(d, es):
            for e in es:
                xcopy(e, d, 0).wait_recv()
                if e in XFWD[d]:
                    xsend(d, e, XFWD[d][e])

        def xfirst(d):
            if d == 0:
                wait_all(xf, lsem.at[L_X])
                for e in range(8):
                    xb[e] = xf[:, e * 128:(e + 1) * 128].astype(BF)
            pl.semaphore_wait(barrier, 2)
            if d == 0:
                for tgt, e in XSEND:
                    xsend(0, e, tgt)
            else:
                xget(d, KORD[d][0:2])
            side_out(0, 1)
            issue_qk(d, (4,))
            issue_qk_last(d)

        def xq(sl):
            return jnp.concatenate([xb[pick([KORD[d][t] for d in range(4)])] for t in sl], axis=1)

        def xwait(sl):
            def fn(d):
                todo = sl if d != 2 else [t + u for t in sl if t % 2 == 0 for u in range(2)]
                xget(d, [KORD[d][t] for t in todo])
            branches(fn, (2, 1, 3) if sl[0] % 2 == 0 else (1, 3))

        for j, sl in enumerate(SWEEP):
            if j == 0:
                branches(xfirst, range(4))
            else:
                xwait(sl)
                if j == 3:
                    side_in(2).start()
            wait_all(w.at[:, pl.ds(sl[0] * 128, len(sl) * 128)], lsem.at[L_QK + j])
            xj = xq(sl)
            for i in range(2):
                t = jnp.dot(xj, w[i, sl[0] * 128:(sl[-1] + 1) * 128].astype(BF),
                            preferred_element_type=F32)
                if j == 0:
                    acc[i] = t
                else:
                    acc[i] += t
        issue_v()
        issue_o(0)
        issue_o(1)
        xwait((6, 7))

        def qk_wait(n):
            wait_all(w.at[n // 2, pl.ds(768, 256), pl.ds(n % 2 * 512, 512)], lsem.at[L_H + n])

        def qk_last(n):
            hf, i = n // 2, n % 2
            c = slice(hf * 512, (hf + 1) * 512)
            t = acc[i, :, c] + jnp.dot(xq((6, 7)), w[hf, 768:1024, i * 512:(i + 1) * 512].astype(BF),
                                       preferred_element_type=F32)
            if i == 0:
                qb[:, c] = (t * QSCALE).astype(BF)
            else:
                kb[:, c] = t.astype(BF)

        def softmax(h):
            c = slice(h * DH, (h + 1) * DH)
            s = lax.dot_general(qb[:, c], kb[:, c], (((1,), (1,)), ((), ())),
                                preferred_element_type=F32)
            p = jnp.exp2(s - jnp.max(s, axis=-1, keepdims=True))
            pb[h] = (p * (1.0 / jnp.sum(p, axis=-1, keepdims=True))).astype(BF)

        def vwait(n):
            wait_all(wv.at[vbox(n)], lsem.at[L_V + n])

        def vproj(n):
            h0, nh, e0, ne, _ = VP[n]
            c = slice(h0 * DH, (h0 + nh) * DH)
            lhs = jnp.concatenate([xb[e] for e in range(e0, e0 + ne)], axis=1)
            t = jnp.dot(lhs, wv[vbox(n)].reshape(ne * 128, nh * DH).astype(BF),
                        preferred_element_type=F32)
            if e0 > 0:
                t = t + vacc[:, c]
            if e0 + ne < 8:
                vacc[:, c] = t
            else:
                vb[:, c] = t.astype(BF)

        def pv(h):
            c = slice(h * DH, (h + 1) * DH)
            ob[:, c] = jnp.dot(pb[h], vb[:, c], preferred_element_type=F32).astype(BF)

        ops = {"Q": qk_wait, "V": vwait, "I": issue_o, "B": side_out,
               "q": qk_last, "s": softmax, "v": vproj, "p": pv}
        for op in STEPS.split():
            ops[op[0]](int(op[1:]))

        def oref(p):
            c, g, r0, n = PIECES[p]
            return out_ref.at[0, pl.ds(g * RG + r0, n), pl.ds(c * CW, CW)]

        def landing(p, m):
            if PLANS[p][m][2] == FULL:
                return oref(p)
            return rbuf.at[rslot[p, m], pl.ds(0, PIECES[p][3])]

        def own(d, buf, p):
            c, g, r0, n = PIECES[p]
            return buf.at[ORD[d].index(c), pos[d, c, g], pl.ds(r0, n)]

        def source(p, m):
            src, _, mask, deps = PLANS[p][m]
            if mask == FULL:
                return oref(p)
            if deps == (-1,):
                return own(src, partb, p)
            if len(deps) == 1:
                return landing(p, deps[0])
            return sbuf.at[sslot[p, m], pl.ds(0, PIECES[p][3])]

        def rcopy(p, m):
            return pltpu.make_async_remote_copy(
                src_ref=source(p, m), dst_ref=landing(p, m),
                send_sem=ssem.at[sslot[p, m]], recv_sem=rsem.at[rslot[p, m]],
                device_id=(PLANS[p][m][1],), device_id_type=pl.DeviceIdType.MESH)

        def run(d, lo, hi):
            for i in range(lo, hi):
                kind, p, m = SEQ[d][i]
                if kind == 5:
                    if i == xdone[d]:
                        for slot, (e, tgt) in enumerate(xsends[d]):
                            xcopy(e, tgt, slot).wait_send()
                    rcopy(p, m).wait_send()
                    continue
                for j in waits[d, i]:
                    rcopy(p, j).wait_recv()
                if sums[d, i]:
                    t = None
                    for j in sums[d, i]:
                        v = own(d, part, p)[...] if j < 0 else landing(p, j)[...].astype(F32)
                        t = v if t is None else t + v
                    (oref(p) if kind == 2 else source(p, m))[...] = t.astype(BF)
                if kind != 2:
                    rcopy(p, m).start()

        hp = PPC // 2
        for b, (k, last) in enumerate(blocks):
            mode = MODES[k]
            halves = (last,) if mode >= 2 else (0, 1)
            for i in halves:
                wait_all(wo.at[k, pl.ds(i * G // 2, G // 2)], lsem.at[L_O + 2 * k + i])
            rows = []
            for j in range(PPC):
                gs = [[g for g in range(PPC) if pos[d, ORD[d][k], g] == j][0] for d in range(4)]
                rows.append(pl.ds(gs[0] * RG if len(set(gs)) == 1
                                  else pl.multiple_of(pick(gs) * RG, RG), RG))
            wh = {i: wo[k, i * G // 2:(i + 1) * G // 2].reshape(D // 2, CW).astype(BF) for i in halves}

            def part_dot(js, i):
                lhs = jnp.concatenate([ob[rows[j], i * 512:(i + 1) * 512] for j in js], axis=0)
                return jnp.dot(lhs, wh[i], preferred_element_type=F32).reshape(len(js), RG, CW)

            def early_sends():
                branches(lambda d: run(d, bpos[d][b] + 1, bpos[d][b] + 1 + early[d, b]),
                         [d for d in BORD if early[d, b]])

            if not last:
                pacc[k % 2] = part_dot(range(PPC), 0)
            elif mode == 0:
                t = part_dot(range(PPC), 0) + part_dot(range(PPC), 1)
                partb[k] = t.astype(BF)
                part[k] = t
            else:
                if mode == 1:
                    ta = part_dot(range(hp), 0) + part_dot(range(hp), 1)
                    tb = part_dot(range(hp, PPC), 1)
                else:
                    t = part_dot(range(PPC), 1)
                    ta, tb = t[0:hp] + pacc[k % 2, 0:hp], t[hp:PPC]
                partb[k, 0:hp] = ta.astype(BF)
                early_sends()
                part[k, 0:hp] = ta
                tb = tb + (part_dot(range(hp, PPC), 0) if mode == 1 else pacc[k % 2, hp:PPC])
                partb[k, hp:PPC] = tb.astype(BF)
                part[k, hp:PPC] = tb
            branches(lambda d: run(d, bpos[d][b] + 1 + early[d, b], bpos[d][b + 1]),
                     [d for d in BORD if bpos[d][b + 1] > bpos[d][b] + 1 + early[d, b]])
            if last and k in OISS:
                issue_o(OISS[k])

    return pl.pallas_call(
        body,
        out_shape=jax.ShapeDtypeStruct((1, S, D), BF),
        in_specs=[pl.BlockSpec(memory_space=pl.ANY)] * 5,
        out_specs=pl.BlockSpec(memory_space=pltpu.VMEM),
        scratch_shapes=[
            pltpu.VMEM((S, D), F32),
            pltpu.VMEM((2, D, D), F32),
            pltpu.VMEM((8, 2, 2, 2, 2, 8, D), F32),
            pltpu.VMEM((NC, G, 2, 2, 8, CW), F32),
            pltpu.VMEM((8, S, 128), BF),
            pltpu.VMEM((2, S, D), F32),
            pltpu.VMEM((S, D), BF),
            pltpu.VMEM((S, D), BF),
            pltpu.VMEM((H, S, S), BF),
            pltpu.VMEM((S, D), F32),
            pltpu.VMEM((S, D), BF),
            pltpu.VMEM((S, D), BF),
            pltpu.VMEM((2, PPC, RG, CW), F32),
            pltpu.VMEM((NC, PPC, RG, CW), F32),
            pltpu.VMEM((NC, PPC, RG, CW), BF),
            pltpu.VMEM((max(nr), RG, CW), BF),
            pltpu.VMEM((max(ns), RG, CW), BF),
            pltpu.SemaphoreType.DMA((L_S + len(SIDE),)),
            pltpu.SemaphoreType.DMA((len(XSEND),)),
            pltpu.SemaphoreType.DMA((8,)),
            pltpu.SemaphoreType.DMA((max(ns),)),
            pltpu.SemaphoreType.DMA((max(nr),)),
        ] + [pltpu.SMEM((rows, 512) if kind == "q" else (1, 2, 2, 2, 8, VP[i][1] * DH), F32)
             for kind, i, rows in SIDE],
        compiler_params=pltpu.CompilerParams(
            collective_id=0, vmem_limit_bytes=48 * 2**20,
            disable_semaphore_checks=True),
    )(x, Wq, Wk, Wv.reshape(8, 2, 2, 2, 2, 8, D), Wo.reshape(G, 2, 2, 8, D))
```
